```python
import numpy as np

kernel_name = "dist_argmax_global_i_m4096_n1024"

def setup_inputs():
    return {"x": np.random.randn(16384, 1024).astype(np.float32)}

def reference(x: np.ndarray) -> np.ndarray:
    idx = np.argmax(x, axis=0).astype(np.float32)
    val = np.max(x, axis=0)
    return np.stack([val, idx], axis=0)
```

```python
import jax
import jax.numpy as jnp
from jax import lax
from jax.experimental import pallas as pl
from jax.experimental.pallas import tpu as pltpu

N_DEV = 4
CHUNK = 256


def _better(v, m):
    return jnp.logical_and(jnp.logical_not(v <= m), m == m)


def pallas_dist_argmax_global_i_m4096_n1024_kernel(
x: jax.Array,
):
    m_per, n = x.shape
    n_chunks = m_per // CHUNK
    groups = CHUNK // 8

    def body(x_hbm, out_ref, buf, comm, copy_sems, send_sems, recv_sems):
        my = lax.axis_index("i")

        copies = []
        for c in range(n_chunks):
            cp = pltpu.make_async_copy(
                x_hbm.at[pl.ds(c * CHUNK, CHUNK)],
                buf.at[pl.ds(c * CHUNK, CHUNK)],
                copy_sems.at[c],
            )
            cp.start()
            copies.append(cp)

        barrier_sem = pltpu.get_barrier_semaphore()
        for d in range(1, N_DEV):
            pl.semaphore_signal(
                barrier_sem, inc=1,
                device_id=((my + d) % N_DEV,),
                device_id_type=pl.DeviceIdType.MESH,
            )

        m = None
        gi = None
        for c in range(n_chunks):
            copies[c].wait()

            def step(g, carry, c=c):
                m_, gi_ = carry
                gg = c * groups + g
                v = buf[pl.ds(pl.multiple_of(gg * 8, 8), 8), :]
                upd = _better(v, m_)
                return jnp.where(upd, v, m_), jnp.where(upd, gg, gi_)

            if c == 0:
                m = buf[pl.ds(0, 8), :]
                gi = jnp.zeros((8, n), jnp.int32)
                m, gi = lax.fori_loop(1, groups, step, (m, gi), unroll=4)
            else:
                m, gi = lax.fori_loop(0, groups, step, (m, gi), unroll=4)

        idx = gi * 8 + lax.broadcasted_iota(jnp.int32, (8, n), 0)
        for shift in (4, 2, 1):
            m2 = pltpu.roll(m, shift, 0)
            i2 = pltpu.roll(idx, shift, 0)
            same = jnp.logical_or(m2 == m, jnp.logical_and(m2 != m2, m != m))
            take = jnp.logical_or(_better(m2, m), jnp.logical_and(same, i2 < idx))
            m = jnp.where(take, m2, m)
            idx = jnp.where(take, i2, idx)

        gidx = (idx + my * m_per).astype(jnp.float32)
        comm[my] = jnp.concatenate([m[0:1, :], gidx[0:1, :]], axis=0)

        pl.semaphore_wait(barrier_sem, N_DEV - 1)

        sends = []
        for d in range(1, N_DEV):
            rdma = pltpu.make_async_remote_copy(
                src_ref=comm.at[my],
                dst_ref=comm.at[my],
                send_sem=send_sems.at[d - 1],
                recv_sem=recv_sems.at[my],
                device_id=((my + d) % N_DEV,),
                device_id_type=pl.DeviceIdType.MESH,
            )
            rdma.start()
            sends.append(rdma)

        for d in range(1, N_DEV):
            src = (my + d) % N_DEV
            pltpu.make_async_remote_copy(
                src_ref=comm.at[src],
                dst_ref=comm.at[src],
                send_sem=send_sems.at[d - 1],
                recv_sem=recv_sems.at[src],
                device_id=(src,),
                device_id_type=pl.DeviceIdType.MESH,
            ).wait_recv()

        bv = comm[0, 0:1, :]
        bi = comm[0, 1:2, :]
        for k in range(1, N_DEV):
            v = comm[k, 0:1, :]
            upd = _better(v, bv)
            bv = jnp.where(upd, v, bv)
            bi = jnp.where(upd, comm[k, 1:2, :], bi)
        out_ref[...] = jnp.concatenate([bv, bi], axis=0)

        for rdma in sends:
            rdma.wait_send()

    return pl.pallas_call(
        body,
        out_shape=jax.ShapeDtypeStruct((2, n), jnp.float32),
        in_specs=[pl.BlockSpec(memory_space=pl.ANY)],
        out_specs=pl.BlockSpec(memory_space=pltpu.VMEM),
        scratch_shapes=[
            pltpu.VMEM((m_per, n), x.dtype),
            pltpu.VMEM((N_DEV, 2, n), jnp.float32),
            pltpu.SemaphoreType.DMA((n_chunks,)),
            pltpu.SemaphoreType.DMA((N_DEV - 1,)),
            pltpu.SemaphoreType.DMA((N_DEV,)),
        ],
        compiler_params=pltpu.CompilerParams(
            collective_id=0,
            vmem_limit_bytes=40 * 1024 * 1024,
        ),
    )(x)
```
